```python
import numpy as np

kernel_name = "dist_ag_xy_y_m1024_n512"

def setup_inputs():
    return {"x": np.random.randn(2048, 512).astype(np.float32)}

def reference(x: np.ndarray) -> np.ndarray:
    return x
```

```python
import jax
import jax.numpy as jnp
from jax import lax
from jax.experimental import pallas as pl
from jax.experimental.pallas import tpu as pltpu

_MESH = pl.DeviceIdType.MESH
_CHUNK = 16
_N_FWD = 29
_LOAD_GROUPS = (1, 3, 25)
_AHEAD = 6
_REST_AT = 16


def pallas_dist_ag_xy_y_m1024_n512_kernel(
    x: jax.Array,
):
    m, n = x.shape
    fwd = _CHUNK * _N_FWD
    direct = m - fwd
    mid = direct - fwd
    n_groups = len(_LOAD_GROUPS)
    group_starts = [sum(_LOAD_GROUPS[:i]) for i in range(n_groups)]

    def kernel_body(x_hbm, o_ref, x_vmem, y_send_sem, mid_sem, x_send_sem, x_recv_sem):
        my_x = lax.axis_index("x")
        my_y = lax.axis_index("y")
        y_nbr = (my_x, 1 - my_y)
        x_nbr = (1 - my_x, my_y)
        mine = pl.multiple_of(my_y * m, m)
        other = pl.multiple_of((1 - my_y) * m, m)
        fwd_own = pl.multiple_of(my_x * direct, _CHUNK)
        fwd_far = pl.multiple_of((1 - my_x) * direct, _CHUNK)

        def remote(row, rows, send_sem, recv_sem, device):
            block = o_ref.at[pl.ds(row, rows)]
            return pltpu.make_async_remote_copy(
                block, block, send_sem, recv_sem, device_id=device, device_id_type=_MESH
            )

        def signal(sem, device):
            pl.semaphore_signal(sem, inc=1, device_id=device, device_id_type=_MESH)

        def store(row, rows):
            o_ref[pl.ds(mine + row, rows), :] = x_vmem[pl.ds(row, rows), :].astype(
                o_ref.dtype
            )

        def pipeline(load_sems, y_recv_sems, relay_sem):
            def load(i, row, rows):
                return pltpu.make_async_copy(
                    x_hbm.at[pl.ds(row, rows)],
                    x_vmem.at[pl.ds(row, rows)],
                    load_sems.at[i],
                )

            loads = {
                s: load(i, fwd_own + s * _CHUNK, g * _CHUNK)
                for i, (s, g) in enumerate(zip(group_starts, _LOAD_GROUPS))
            }
            loads[_N_FWD] = load(n_groups, fwd, mid)
            rest = load(n_groups + 1, fwd_far, fwd)

            loads[0].start()
            barrier = pltpu.get_barrier_semaphore()
            signal(barrier, y_nbr)
            pl.when(my_y == 0)(lambda: signal(barrier, x_nbr))
            for s in list(loads)[1:]:
                loads[s].start()

            def send(c):
                row, rows = (fwd_own + c * _CHUNK, _CHUNK) if c < _N_FWD else (fwd, mid)
                if c == 2:
                    rest.start()
                if c in loads:
                    loads[c].wait()
                store(row, rows)
                if c == 0:
                    pl.when(my_y == 0)(lambda: pl.semaphore_wait(barrier, 2))
                    pl.when(my_y == 1)(lambda: pl.semaphore_wait(barrier, 1))
                recv_sem = y_recv_sems.at[c] if c < _N_FWD else mid_sem
                remote(mine + row, rows, y_send_sem, recv_sem, y_nbr).start()
                if c == 0:
                    pl.when(my_y == 0)(lambda: signal(relay_sem, x_nbr))

            for c in range(_AHEAD):
                send(c)
            pl.semaphore_wait(relay_sem, 1)
            pl.when(my_y == 0)(lambda: signal(relay_sem, y_nbr))

            for c in range(_N_FWD):
                row = other + fwd_own + c * _CHUNK
                remote(row, _CHUNK, y_send_sem, y_recv_sems.at[c], y_nbr).wait_recv()
                remote(row, _CHUNK, x_send_sem, x_recv_sem, x_nbr).start()
                if c + _AHEAD <= _N_FWD:
                    send(c + _AHEAD)
                if c == _REST_AT:
                    rest.wait()
                    store(fwd_far, fwd)

        pl.run_scoped(
            pipeline,
            pltpu.SemaphoreType.DMA((n_groups + 2,)),
            pltpu.SemaphoreType.DMA((_N_FWD,)),
            pltpu.SemaphoreType.REGULAR,
        )

        sent = pl.multiple_of(mine + my_x * fwd, _CHUNK)
        remote(other + fwd, mid, y_send_sem, mid_sem, y_nbr).wait_recv()
        remote(sent, direct, y_send_sem, mid_sem, y_nbr).wait_send()
        remote(other + fwd_own, fwd, x_send_sem, x_recv_sem, x_nbr).wait_send()
        remote(other + fwd_far, fwd, x_send_sem, x_recv_sem, x_nbr).wait_recv()

    return pl.pallas_call(
        kernel_body,
        out_shape=pltpu.VMEM((2 * m, n), jnp.bfloat16),
        in_specs=[pl.BlockSpec(memory_space=pltpu.HBM)],
        out_specs=pl.BlockSpec(memory_space=pltpu.VMEM),
        scratch_shapes=[
            pltpu.VMEM((m, n), x.dtype),
            pltpu.SemaphoreType.DMA,
            pltpu.SemaphoreType.DMA,
            pltpu.SemaphoreType.DMA,
            pltpu.SemaphoreType.DMA,
        ],
        compiler_params=pltpu.CompilerParams(collective_id=0),
    )(x)
```
